```python
import numpy as np

kernel_name = "dist_sparse_attn_strided_htp_bs_b2_sq256_skv256_hq4_dh64"

def setup_inputs():
    x = np.random.randn(8, 256, 512).astype(np.float32)
    Wq = np.random.randn(512, 1024).astype(np.float32) * 0.02
    K_ext = np.random.randn(8, 256, 16, 64).astype(np.float32)
    V_ext = np.random.randn(8, 256, 16, 64).astype(np.float32)
    Wo = np.random.randn(1024, 512).astype(np.float32) * 0.02
    return {"x": x, "Wq": Wq, "K_ext": K_ext, "V_ext": V_ext, "Wo": Wo}

def reference(x, Wq, K_ext, V_ext, Wo):
    B, Sq, Skv, Hq, Dh = 8, 256, 256, 16, 64
    Q = (x @ Wq).reshape(B, Sq, Hq, Dh)
    qb = (np.arange(Sq) // 64)[:, None]
    kb = (np.arange(Skv) // 64)[None, :]
    mask = (qb == kb) | ((kb % 4) == (qb % 4))
    scores = np.einsum('bihd,bjhd->bhij', Q, K_ext).astype(np.float32) * 0.125
    scores = np.where(mask[None, None, :, :], scores, -1e9)
    scores_max = scores.max(axis=-1, keepdims=True)
    w = np.exp(scores - scores_max)
    row_keep = mask.any(axis=1)
    w_sum = np.where(row_keep[None, None, :, None], w.sum(axis=-1, keepdims=True), 1.0)
    w = w / w_sum
    w = np.where(row_keep[None, None, :, None], w, 0.0)
    ctx = np.einsum('bhij,bjhd->bihd', w, V_ext).reshape(B, Sq, Hq * Dh)
    return ctx @ Wo
```

```python
import contextlib
import math

import jax
import jax.numpy as jnp
from jax import lax
from jax.experimental import pallas as pl
from jax.experimental.pallas import tpu as pltpu

F32, BF16 = jnp.float32, jnp.bfloat16
MESH = pl.DeviceIdType.MESH
NT = (((1,), (1,)), ((), ()))
K_SCALE = 0.125 * math.log2(math.e)
OWN, NA, NB, DG = 0, 1, 2, 3


def make(out_dtype=BF16, trace=False, **cp):
    scope = jax.named_scope if trace else (lambda name: contextlib.nullcontext())

    def body(x_hbm, wq_hbm, kt_hbm, vt_hbm, wo_hbm, out_ref,
             xf, wqf, wof, ktf, vtf, xb, wq, wo, kb, vb, ctx, acc,
             lsem, ssem, rsem, hsem):
        me = lax.axis_index("i")
        na, nb = me ^ 1, me ^ 3
        bar = pltpu.get_barrier_semaphore()

        ld_wq0 = pltpu.make_async_copy(wq_hbm.at[pl.ds(0, 128)], wqf.at[pl.ds(0, 128)], lsem.at[0])
        ld_wq1 = pltpu.make_async_copy(wq_hbm.at[pl.ds(128, 384)], wqf.at[pl.ds(128, 384)], lsem.at[1])
        ld_wo = pltpu.make_async_copy(wo_hbm, wof, lsem.at[2])
        ld_x = pltpu.make_async_copy(x_hbm, xf, lsem.at[3])
        ld_wq0.start()

        def signal(sem, dev):
            pl.semaphore_signal(sem, inc=1, device_id=(dev,), device_id_type=MESH)

        @pl.when(me != 2)
        def _():
            signal(bar, na)
            signal(bar, nb)

        ld_wq1.start()
        ld_wo.start()
        ld_x.start()

        @pl.when(me == 2)
        def _():
            pl.semaphore_wait(bar, 2)
            signal(hsem, na)
            signal(hsem, nb)

        ld_k, ld_v = [], []
        for s, dev in enumerate((me, na, nb, me ^ 2)):
            src = (pl.ds(2 * me, 2), pl.ds(pl.multiple_of(dev * 256, 256), 256))
            ld_k.append(pltpu.make_async_copy(kt_hbm.at[src], ktf.at[s], lsem.at[4 + s]))
            ld_v.append(pltpu.make_async_copy(vt_hbm.at[src], vtf.at[s], lsem.at[8 + s]))

        sends = []

        def rcopy(src, dst, link, k):
            return pltpu.make_async_remote_copy(
                src, dst, ssem.at[link], rsem.at[k],
                device_id=((na, nb)[link],), device_id_type=MESH)

        top, rest = pl.ds(0, 128), pl.ds(128, 384)
        q_first0 = [rcopy(wq.at[OWN, l, top], wq.at[NA + l, l, top], l, 0 + l) for l in (0, 1)]
        q_first1 = [rcopy(wq.at[OWN, l, rest], wq.at[NA + l, l, rest], l, 2 + l) for l in (0, 1)]
        q_second = [rcopy(wq.at[OWN, 1 - l], wq.at[NA + l, 1 - l], l, 4 + l) for l in (0, 1)]
        o_first = [rcopy(wo.at[OWN, l], wo.at[NA + l, l], l, 6 + l) for l in (0, 1)]
        q_fwd = [rcopy(wq.at[NB - l, 1 - l], wq.at[DG, 1 - l], l, 8 + l) for l in (0, 1)]
        o_second = [rcopy(wo.at[OWN, 1 - l], wo.at[NA + l, 1 - l], l, 10 + l) for l in (0, 1)]
        o_fwd = [[rcopy(wo.at[NB - l, 1 - l, c], wo.at[DG, 1 - l, c], l, 12 + 2 * c + l) for l in (0, 1)]
                 for c in range(4)]
        late = (3, 1)

        def start_early(cps):
            for l in (0, 1):
                pl.when(me != late[l])(cps[l].start)

        with scope("wq0"):
            ld_wq0.wait()
            for h in (0, 1):
                wq[OWN, h, 0:128] = wqf[0:128, h * 128:(h + 1) * 128].astype(BF16)
        with scope("bar"):
            pl.when(me == 0)(lambda: pl.semaphore_wait(bar, 2))
            pl.when((me & 1) == 1)(lambda: pl.semaphore_wait(bar, 1))
            start_early(q_first0)
        with scope("wq1"):
            ld_wq1.wait()
            for h in (0, 1):
                wq[OWN, h, 128:512] = wqf[128:512, h * 128:(h + 1) * 128].astype(BF16)
            start_early(q_first1)
            start_early(q_second)
        for s in range(4):
            ld_k[s].start()
            ld_v[s].start()
        with scope("hs"):
            for l in (0, 1):
                @pl.when(me == late[l])
                def _():
                    pl.semaphore_wait(hsem, 1)
                    q_first0[l].start()
                    q_first1[l].start()
                    q_second[l].start()
        with scope("wo"):
            ld_wo.wait()
            for h in (0, 1):
                for c in range(4):
                    wo[OWN, h, c] = wof[h * 128:(h + 1) * 128, c * 128:(c + 1) * 128].astype(BF16)
            for l in (0, 1):
                o_first[l].start()

        lane = lax.broadcasted_iota(jnp.int32, (128, 128), 1)
        row = lax.broadcasted_iota(jnp.int32, (128, 128), 0)
        diag = (lane < 64) == (row < 64)
        lo = lax.broadcasted_iota(jnp.int32, (64, 128), 1) < 64
        lo1 = lax.broadcasted_iota(jnp.int32, (1, 128), 1) < 64

        def kv_prep(s):
            ld_k[s].wait()
            ld_v[s].wait()
            for g in range(4):
                b, cols = g // 2, slice((g % 2) * 128, (g % 2 + 1) * 128)
                for p in range(2):
                    rows = slice(p * 128, (p + 1) * 128)
                    t = (ktf[s, b, rows, cols] * K_SCALE).T
                    kb[s, p, g] = jnp.concatenate(
                        [jnp.where(lo, t[0:64], t[64:128]), jnp.where(lo, t[64:128], t[0:64])], 0).astype(BF16)
                    vb[s, p, g] = vtf[s, b, rows, cols].astype(BF16)

        def softmax_t(s):
            e = jnp.exp2(s - jnp.max(s, axis=0, keepdims=True))
            return e, jnp.sum(e, axis=0, keepdims=True)

        def attend(pairs):
            w = jnp.concatenate([wq[s, p] for s, p in pairs], axis=1)
            q = jnp.dot(xb[...], w, preferred_element_type=F32)
            tiles = [(i, g) for g in range(4) for i in range(len(pairs))]
            sc, pr = {}, {}
            for i, g in tiles:
                s, p = pairs[i]
                qt = q[g * 128:(g + 1) * 128, i * 128:(i + 1) * 128]
                sc[i, g] = (
                    lax.dot_general(kb[s, p, g, 0:64], jnp.where(diag, qt, 0.).astype(BF16), NT,
                                    preferred_element_type=F32),
                    lax.dot_general(kb[s, p, g, 64:128], jnp.where(diag, 0., qt).astype(BF16), NT,
                                    preferred_element_type=F32))
            for i, g in tiles:
                (p1, l1), (p2, l2) = softmax_t(sc[i, g][0]), softmax_t(sc[i, g][1])
                r0 = jnp.concatenate([jnp.where(lo, p1, 0.), jnp.where(lo, 0., p2)], 0).astype(BF16)
                r1 = jnp.concatenate([jnp.where(lo, p2, 0.), jnp.where(lo, 0., p1)], 0).astype(BF16)
                pr[i, g] = (r0, r1, 1.0 / jnp.where(lo1, l1, l2), 1.0 / jnp.where(lo1, l2, l1))
            for i, g in tiles:
                s, p = pairs[i]
                r0, r1, i0, i1 = pr[i, g]
                c0 = jnp.dot(vb[s, p, g, 0:64], r0, preferred_element_type=F32) * i0
                c1 = jnp.dot(vb[s, p, g, 64:128], r1, preferred_element_type=F32) * i1
                ctx[s, p, g * 128:(g + 1) * 128] = jnp.concatenate([c0, c1], 0).astype(BF16).T

        def project(pairs, slabs):
            lhs = jnp.concatenate([ctx[s, p] for s, p in pairs], axis=1)
            rhs = jnp.concatenate(
                [jnp.concatenate([wo[s, p, c] for c in slabs], axis=1) for s, p in pairs], axis=0)
            return jnp.dot(lhs, rhs, preferred_element_type=F32)

        with scope("x"):
            ld_x.wait()
            xb[...] = xf[...].astype(BF16)
        with scope("kv0"):
            kv_prep(OWN)
        with scope("own"):
            attend([(OWN, 0), (OWN, 1)])
            acc[...] = project([(OWN, 0), (OWN, 1)], range(4))
        with scope("w_q1"):
            for l in (0, 1):
                q_first0[l].wait_recv()
                q_first1[l].wait_recv()
            for l in (0, 1):
                q_fwd[l].start()
                o_second[l].start()
        with scope("kv12"):
            kv_prep(NA)
            kv_prep(NB)
        with scope("att1"):
            attend([(NA, 0), (NB, 1)])
        with scope("kv3"):
            kv_prep(DG)
        with scope("w_q2"):
            for l in (0, 1):
                q_second[l].wait_recv()
        with scope("att2"):
            attend([(NA, 1), (NB, 0)])
        with scope("w_o1"):
            for l in (0, 1):
                o_first[l].wait_recv()
            for c in range(4):
                for l in (0, 1):
                    o_fwd[c][l].start()
        with scope("pr1"):
            acc[...] += project([(NA, 0), (NB, 1)], range(4))
        with scope("w_q3"):
            for l in (0, 1):
                q_fwd[l].wait_recv()
        with scope("att3"):
            attend([(DG, 0), (DG, 1)])
        with scope("w_o2"):
            for l in (0, 1):
                o_second[l].wait_recv()
        with scope("pr2"):
            acc[...] += project([(NA, 1), (NB, 0)], range(4))
        for c in range(4):
            with scope(f"w_f{c}"):
                for l in (0, 1):
                    o_fwd[c][l].wait_recv()
            with scope(f"f{c}"):
                cols = slice(c * 128, (c + 1) * 128)
                out_ref[:, cols] = (acc[:, cols] + project([(DG, 0), (DG, 1)], [c])).astype(out_ref.dtype)
        with scope("w_send"):
            for l in (0, 1):
                for cps in (q_first0, q_first1, q_second, o_first, q_fwd, o_second, *o_fwd):
                    cps[l].wait_send()

    def kernel(x, Wq, K_ext, V_ext, Wo):
        kt = jnp.transpose(K_ext, (0, 2, 3, 1)).reshape(8, 1024, 256)
        vt = jnp.transpose(V_ext, (0, 2, 3, 1)).reshape(8, 1024, 256)
        hbm = pl.BlockSpec(memory_space=pltpu.HBM)
        out = pl.pallas_call(
            body,
            out_shape=jax.ShapeDtypeStruct((512, 512), out_dtype),
            in_specs=[hbm] * 5,
            out_specs=pl.BlockSpec(memory_space=pltpu.VMEM),
            scratch_shapes=[
                pltpu.VMEM((512, 512), F32), pltpu.VMEM((512, 256), F32), pltpu.VMEM((256, 512), F32),
                pltpu.VMEM((4, 2, 256, 256), F32), pltpu.VMEM((4, 2, 256, 256), F32),
                pltpu.VMEM((512, 512), BF16),
                pltpu.VMEM((4, 2, 512, 128), BF16), pltpu.VMEM((4, 2, 4, 128, 128), BF16),
                pltpu.VMEM((4, 2, 4, 128, 128), BF16), pltpu.VMEM((4, 2, 4, 128, 128), BF16),
                pltpu.VMEM((4, 2, 512, 128), BF16), pltpu.VMEM((512, 512), F32),
                pltpu.SemaphoreType.DMA((12,)), pltpu.SemaphoreType.DMA((2,)), pltpu.SemaphoreType.DMA((20,)),
                pltpu.SemaphoreType.REGULAR,
            ],
            compiler_params=pltpu.CompilerParams(collective_id=0, vmem_limit_bytes=48 * 1024 * 1024, **cp),
        )(x.reshape(512, 512), Wq, kt, vt, Wo)
        return out.reshape(2, 256, 512)

    return kernel


_kernel = make(disable_semaphore_checks=True)


def pallas_dist_sparse_attn_strided_htp_bs_b2_sq256_skv256_hq4_dh64_kernel(x, Wq, K_ext, V_ext, Wo):
    return _kernel(x, Wq, K_ext, V_ext, Wo)
```

```python
import functools
import math

import jax
import jax.numpy as jnp
from jax import lax
from jax.experimental import pallas as pl
from jax.experimental.pallas import tpu as pltpu

F32, BF16, I32 = jnp.float32, jnp.bfloat16, jnp.int32
MESH = pl.DeviceIdType.MESH
NT_DIMS = (((1,), (1,)), ((), ()))
K_SCALE = 0.125 * math.log2(math.e)

OWN, NA, NB, FAR = 0, 1, 2, 3
WQ, WO = 0, 1
LINKS = (0, 1)
PHASES = (((OWN, 0), (OWN, 1)), ((NA, 0), (NB, 1)), ((NA, 1), (NB, 0)), ((FAR, 0), (FAR, 1)))
WQ_PIECES = ((0, 32), (32, 32), (64, 64), (128, 128), (256, 256))


def _i32(v):
    return v - (1 << 32) if v >> 31 else v


def _bytes(v):
    return _i32(v * 0x01010101)


def _shr(v, n):
    return lax.shift_right_logical(v, jnp.broadcast_to(jnp.asarray(n, I32), v.shape))


SM_MASK, EXP_MASK = _i32(0x807F807F), 0x7F807F80
QUADS, PLANES, QUEUE = 32, 4, 8
VALUES = 4 * QUADS
GROUP = 6
FIRST_BIT, LAST_BIT = 2, 32 * (QUEUE + 1)

SM_ROWS = 8 * QUADS // 2
CODE_ROW, CODE_ROWS = 2 * SM_ROWS, 8 * (QUEUE + PLANES)
WIRE_ROWS = CODE_ROW + CODE_ROWS


def _word_range(i):
    return (FIRST_BIT + i) // 32, min(FIRST_BIT + 32 * (i // GROUP), LAST_BIT - (VALUES - i)) // 32


def _partner(v):
    return jnp.concatenate([pltpu.roll(v[r:r + 8], 4, 0) for r in range(0, v.shape[0], 8)], axis=0)


def _reverse_bits(v):
    for n, mask in ((1, 0x55555555), (2, 0x33333333), (4, 0x0F0F0F0F), (8, 0x00FF00FF)):
        v = (_shr(v, n) & mask) | ((v & mask) << n)
    return _shr(v, 16) | (v << 16)


def _at_most(v, bound):
    return (_bytes(0x80 + bound) - v) & _bytes(0x80)


def _spread(byte):
    byte = byte | (byte << 8)
    return byte | (byte << 16)


def _encode(quads, top):
    total = functools.reduce(jnp.add, [e & 0x00FF00FF for e in quads])
    total = jnp.sum(((total & 0xFFFF) + _shr(total, 16)).astype(F32), axis=0, keepdims=True)
    ref = jnp.maximum(top, jnp.minimum((total * (1.0 / 512) + 3.5).astype(I32), 255))
    ref = jnp.broadcast_to(ref, (8, 128))
    ref4 = _spread(ref)
    zero = jnp.zeros((8, 128), I32)
    planes, queue, lengths, seen = [zero] * PLANES, [zero] * (QUEUE + 1), [], zero
    for i, e in enumerate(quads):
        v = ref4 - e
        le0, le1, le4, le8 = (_at_most(v, b) for b in (0, 1, 4, 8))
        rank = v + _shr(le0, 4) + _shr(le0, 6) + _shr(le0 ^ le1, 5) - _shr(le4, 7) - _shr(le8, 7)
        planes[i // 8] = planes[i // 8] | ((rank & _bytes(1)) << (i % 8))
        n = (_shr(rank, 1) & _bytes(0x7F)) + _bytes(1)
        seen = seen | v | (n << 1)
        lengths += [n & 31, _shr(n, 8) & 31, _shr(n, 16) & 31, _shr(n, 24) & 31]
    pos, bad = zero + FIRST_BIT, (seen & _bytes(0xC0)) != 0
    for i in range(0, VALUES, GROUP):
        bits, used = jnp.ones((8, 128), I32), lengths[i]
        for n in lengths[i + 1:i + GROUP]:
            bits, used = (bits << n) | 1, used + n
        bad = bad | (used > 32)
        bits = bits << ((32 - used) & 31)
        k, s = _shr(pos, 5), pos & 31
        head, rest = _shr(bits, s), (bits << 1) << (31 - s)
        k0, k1 = _word_range(i)
        here = {kk: k == kk for kk in range(k0, k1 + 1)}
        for kk in range(k0, min(k1 + 2, QUEUE + 1)):
            part = jnp.where(here[kk - 1], rest, 0) if kk > k0 else zero
            queue[kk] = queue[kk] | (jnp.where(here[kk], head, part) if kk <= k1 else part)
        pos = pos + used
    bad = bad | (pos > LAST_BIT) | (pos + _partner(pos) > 64 * QUEUE)
    unfit = jnp.max(jnp.where(bad, 1.0, 0.0)) > 0.0
    sub = lax.broadcasted_iota(I32, (8, 128), 0)
    queue[0] = queue[0] | ((_shr(ref, sub) & 1) << 30)
    queue[QUEUE - 1] = queue[QUEUE - 1] | _reverse_bits(_partner(queue[QUEUE]))
    flag = -unfit.astype(I32)
    return [word | flag for word in queue[:QUEUE]] + planes, unfit


def _decode(words, emit):
    queue, planes = words[:QUEUE], words[QUEUE:]
    queue = queue + [_reverse_bits(_partner(queue[-1]))]
    pos = jnp.full(queue[0].shape, FIRST_BIT, I32)
    sub = lax.broadcasted_iota(I32, (8, 128), 0)
    refs = []
    for r in range(0, pos.shape[0], 8):
        ref = jnp.sum(((_shr(queue[0][r:r + 8], 30) & 1) << sub).astype(F32), axis=0, keepdims=True)
        refs.append(jnp.broadcast_to(ref.astype(I32), (8, 128)))
    ref4 = _spread(jnp.concatenate(refs, axis=0))
    for i in range(VALUES):
        if i % GROUP == 0:
            k0, k1 = _word_range(i)
            k, s = _shr(pos, 5), pos & 31
            cur, nxt = queue[k0], queue[k0 + 1]
            for kk in range(k0 + 1, k1 + 1):
                here = k == kk
                cur = jnp.where(here, queue[kk], cur)
                if kk < QUEUE:
                    nxt = jnp.where(here, queue[kk + 1], nxt)
            window = (cur << s) | _shr(_shr(nxt, 1), 31 - s)
            pos = pos + GROUP
        z = lax.clz(window)
        window, pos = (window << 1) << z, pos + z
        rank = z << 1 if i % 4 == 0 else rank | (z << (8 * (i % 4) + 1))
        if i % 4 == 3:
            q = i // 4
            rank = rank | (_shr(planes[q // 8], q % 8) & _bytes(1))
            le2, le3, le7, le8 = (_at_most(rank, b) for b in (2, 3, 7, 8))
            v = rank + _shr(le3, 7) + _shr(le7, 7) - _shr(le2 ^ le3, 5) - _shr(le7 ^ le8, 4)
            emit(q, ref4 - v)


def _body(x_hbm, wq_hbm, kt_hbm, vt_hbm, wo_hbm, out_ref,
          xf, wqf, wof, ktf, vtf, xb, own, wire, expo, plain, q_own, kb, vb, ctx_t, ctx, acc,
          load_sem, send_sem, recv_sem, plain_sem, entry_sem):
    me = lax.axis_index("i")
    nbr = (me ^ 1, me ^ 3)
    barrier = pltpu.get_barrier_semaphore()

    def start(*groups):
        for group in groups:
            for dma in group:
                dma.start()

    def arrived(*groups):
        for group in groups:
            for dma in group:
                dma.wait_recv()

    def tell_neighbours(sem):
        for dev in nbr:
            pl.semaphore_signal(sem, inc=1, device_id=(dev,), device_id_type=MESH)

    ld_wq = [pltpu.make_async_copy(wq_hbm.at[pl.ds(r, n)], wqf.at[pl.ds(r, n)], load_sem.at[6 + i])
             for i, (r, n) in enumerate(WQ_PIECES)]
    ld_wo = pltpu.make_async_copy(wo_hbm, wof, load_sem.at[0])
    ld_x = pltpu.make_async_copy(x_hbm, xf, load_sem.at[1])
    ld_wq[0].start()
    pl.when(me != 2)(lambda: tell_neighbours(barrier))
    start(ld_wq[1:], [ld_wo, ld_x])

    @pl.when(me == 2)
    def _():
        pl.semaphore_wait(barrier, 2)
        tell_neighbours(entry_sem)

    owner = (me, *nbr, me ^ 2)
    ld_kv = []
    for i, pairs in enumerate(PHASES):
        ld_kv.append([])
        for j, (s, h) in enumerate(pairs):
            src = (pl.ds(2 * me, 2), pl.ds(pl.multiple_of(owner[s] * 256 + h * 128, 128), 128))
            ld_kv[i] += [pltpu.make_async_copy(kt_hbm.at[src], ktf.at[i, j], load_sem.at[2 + i]),
                         pltpu.make_async_copy(vt_hbm.at[src], vtf.at[i, j], load_sem.at[2 + i])]

    def remote(k, m, relay, first_row, rows):
        group = []
        for l in LINKS:
            src, dst = (NB - l, FAR) if relay else (OWN, NA + l)
            span = pl.ds(first_row[l], rows)
            group.append(pltpu.make_async_remote_copy(
                wire.at[src, m, span], wire.at[dst, m, span], send_sem.at[l], recv_sem.at[2 * k + l],
                device_id=(nbr[l],), device_id_type=MESH))
        return group

    def first(r=0):
        return (r, SM_ROWS + r)

    def second(r=0):
        return (SM_ROWS + r, r)

    q_first_parts = [remote(0, WQ, False, first(r // 4), n // 4) for r, n in WQ_PIECES]
    q_first = remote(0, WQ, False, first(), SM_ROWS)
    q_second_parts = [remote(1, WQ, False, second(), 32), remote(1, WQ, False, second(32), SM_ROWS - 32)]
    q_second = remote(1, WQ, False, second(), SM_ROWS)
    q_code, o_code = (remote(2 + m, m, False, (CODE_ROW, CODE_ROW), CODE_ROWS) for m in (WQ, WO))
    o_first = remote(4, WO, False, first(), SM_ROWS)
    far_q_code, far_o_code = (
        remote(5 + m, m, True, (CODE_ROW, CODE_ROW + CODE_ROWS // 2), CODE_ROWS // 2) for m in (WQ, WO))
    far_q = remote(7, WQ, True, second(), SM_ROWS)
    o_second = [remote(8 + i, WO, False, second(64 * i), 64) for i in range(2)]
    far_o = [remote(10 + t, WO, True, second(32 * t), 32) for t in range(4)]

    def plain_own(m, l):
        return pltpu.make_async_remote_copy(
            expo.at[OWN, m], plain.at[l, m], plain_sem.at[8 * m + l], plain_sem.at[8 * m + 2 + l],
            device_id=(nbr[l],), device_id_type=MESH)

    def plain_far(m, l):
        span = pl.ds(SM_ROWS * l, SM_ROWS)
        return pltpu.make_async_remote_copy(
            plain.at[1 - l, m, span], plain.at[2, m, span],
            plain_sem.at[8 * m + 4 + l], plain_sem.at[8 * m + 6 + l],
            device_id=(nbr[l],), device_id_type=MESH)

    def split(m, h, r, block):
        n = block.shape[0]
        own[m, h, pl.ds(r, n)] = block.astype(BF16)
        w = pltpu.bitcast(own[m, h, pl.ds(r, n)], I32)
        for i in range(n // 32):
            a, b = w[16 * i:16 * i + 8], w[16 * i + 8:16 * i + 16]
            rows, sm = pl.ds(SM_ROWS * h + r // 4 + 8 * i, 8), b & SM_MASK
            wire[OWN, m, rows] = (a & SM_MASK) | (sm << 8) | _shr(sm, 24)
            expo[OWN, m, rows] = (_shr(a, 7) & 0x00FF00FF) | ((b << 1) & _i32(0xFF00FF00))

    def pack(m, src):
        top = jnp.max(jnp.abs(src[...]), axis=0, keepdims=True)
        top = functools.reduce(jnp.maximum, [top[:, c:c + 128] for c in range(0, top.shape[1], 128)])
        top = _shr(pltpu.bitcast(top.astype(BF16).astype(F32), I32), 23) & 255
        words, unfit = _encode([expo[OWN, m, pl.ds(8 * i, 8)] for i in range(QUADS)], top)
        wire[OWN, m, pl.ds(CODE_ROW, CODE_ROWS)] = jnp.concatenate(words, axis=0)
        return unfit

    def unpack(slots, m):
        def emit(i, quad):
            for j, s in enumerate(slots):
                expo[s, m, pl.ds(8 * i, 8)] = quad[8 * j:8 * j + 8]

        _decode([jnp.concatenate([wire[s, m, pl.ds(r, 8)] for s in slots], axis=0)
                 for r in range(CODE_ROW, WIRE_ROWS, 8)], emit)

    def is_unfit(s, m):
        return wire[s, m, pl.ds(CODE_ROW, 8)][0, 0] < 0

    def use_plain_near(m):
        unfit = [is_unfit(NA + l, m) for l in LINKS]
        for l in LINKS:
            @pl.when(unfit[l])
            def _():
                plain_own(m, l).wait_recv()
                relay = plain_far(m, 1 - l)
                relay.start()
                expo[NA + l, m] = plain[l, m]
                relay.wait_send()

    def use_plain_far(m):
        @pl.when(is_unfit(FAR, m))
        def _():
            arrived([plain_far(m, l) for l in LINKS])
            expo[FAR, m] = plain[2, m]

    def weight(s, m, h, t):
        if s == OWN:
            return own[m, h, pl.ds(128 * t, 128)]
        words = []
        for r in range(SM_ROWS * h + 32 * t, SM_ROWS * h + 32 * t + 32, 8):
            p, e = wire[s, m, pl.ds(r, 8)], expo[s, m, pl.ds(r, 8)]
            words += [(p & SM_MASK) | ((e << 7) & EXP_MASK),
                      ((_shr(p, 8) | (p << 24)) & SM_MASK) | (_shr(e, 1) & EXP_MASK)]
        return pltpu.bitcast(jnp.concatenate(words, axis=0), BF16)

    @pl.when(me == 0)
    def _():
        start(ld_kv[0])
        pl.semaphore_wait(barrier, 2)

    pl.when((me & 1) == 1)(lambda: pl.semaphore_wait(barrier, 1))
    faces_2 = (3, 1)
    for i, (r, n) in enumerate(WQ_PIECES):
        ld_wq[i].wait()
        for h in range(2):
            split(WQ, h, r, wqf[r:r + n, h * 128:(h + 1) * 128])
        for l in LINKS:
            pl.when(me != faces_2[l])(q_first_parts[i][l].start)
    pl.when(me != 0)(lambda: start(ld_kv[0]))
    for l in LINKS:
        @pl.when(me == faces_2[l])
        def _():
            pl.semaphore_wait(entry_sem, 1)
            start([group[l] for group in q_first_parts])

    start(q_second_parts[0])
    unfit_q = pack(WQ, wqf)
    start(q_code, q_second_parts[1])
    ld_wo.wait()
    for h in range(2):
        for t in range(4):
            split(WO, h, 128 * t, wof[h * 128:(h + 1) * 128, t * 128:(t + 1) * 128])
    unfit_o = pack(WO, wof)
    start(o_code, o_first, *ld_kv[1:])
    for m, unfit in ((WQ, unfit_q), (WO, unfit_o)):
        @pl.when(unfit)
        def _():
            copies = [plain_own(m, l) for l in LINKS]
            start(copies)
            for dma in copies:
                dma.wait_send()

    diag = ((lax.broadcasted_iota(I32, (128, 128), 1) < 64)
            == (lax.broadcasted_iota(I32, (128, 128), 0) < 64))
    left = lax.broadcasted_iota(I32, (64, 128), 1) < 64
    left_row = lax.broadcasted_iota(I32, (1, 128), 1) < 64
    tiles = [(j, g) for g in range(4) for j in range(2)]

    def kv_wait(i):
        for dma in ld_kv[i]:
            dma.wait()

    def kv_prep(i):
        for j, g in tiles:
            b, cols = g // 2, slice((g % 2) * 128, (g % 2 + 1) * 128)
            k = (ktf[i, j, b, :, cols] * K_SCALE).T
            kb[i, j, g] = jnp.concatenate(
                [jnp.where(left, k[0:64], k[64:128]), jnp.where(left, k[64:128], k[0:64])], 0).astype(BF16)
            vb[i, j, g] = vtf[i, j, b, :, cols].astype(BF16)

    def query(i):
        w = jnp.concatenate(
            [jnp.concatenate([weight(s, WQ, h, t) for t in range(4)], axis=0) for s, h in PHASES[i]], axis=1)
        return jnp.dot(xb[...], w, preferred_element_type=F32)

    def softmax_terms(s):
        e = jnp.exp2(s - jnp.max(s, axis=0, keepdims=True))
        return e, jnp.sum(e, axis=0, keepdims=True)

    def attend(i, q):
        scores, probs = {}, {}
        for j, g in tiles:
            qt = q[g * 128:(g + 1) * 128, j * 128:(j + 1) * 128]
            scores[j, g] = (
                lax.dot_general(kb[i, j, g, 0:64], jnp.where(diag, qt, 0.).astype(BF16), NT_DIMS,
                                preferred_element_type=F32),
                lax.dot_general(kb[i, j, g, 64:128], jnp.where(diag, 0., qt).astype(BF16), NT_DIMS,
                                preferred_element_type=F32))
        for j, g in tiles:
            (p1, l1), (p2, l2) = softmax_terms(scores[j, g][0]), softmax_terms(scores[j, g][1])
            probs[j, g] = (
                jnp.concatenate([jnp.where(left, p1, 0.), jnp.where(left, 0., p2)], 0).astype(BF16),
                jnp.concatenate([jnp.where(left, p2, 0.), jnp.where(left, 0., p1)], 0).astype(BF16),
                1.0 / jnp.where(left_row, l1, l2), 1.0 / jnp.where(left_row, l2, l1))
        for j, g in tiles:
            head0, head1, inv0, inv1 = probs[j, g]
            tile = jnp.concatenate(
                [jnp.dot(vb[i, j, g, 0:64], head0, preferred_element_type=F32) * inv0,
                 jnp.dot(vb[i, j, g, 64:128], head1, preferred_element_type=F32) * inv1], 0).astype(BF16)
            if i == 0:
                ctx[i, g * 128:(g + 1) * 128, j * 128:(j + 1) * 128] = tile.T
            else:
                ctx_t[j, g] = tile

    def finish(i):
        for j, g in tiles:
            ctx[i, g * 128:(g + 1) * 128, j * 128:(j + 1) * 128] = ctx_t[j, g].T

    def project(i, slabs, rows=slice(None)):
        w = jnp.concatenate(
            [jnp.concatenate([weight(s, WO, h, t) for t in slabs], axis=1) for s, h in PHASES[i]], axis=0)
        return jnp.dot(ctx[i, rows], w, preferred_element_type=F32)

    ld_x.wait()
    xb[...] = xf[...].astype(BF16)
    q_own[...] = query(0)

    kv_wait(0)
    kv_prep(0)
    attend(0, q_own)

    arrived(q_first, q_code)
    start(far_q_code, far_q)
    unpack((NA, NB), WQ)
    acc[...] = project(0, range(4))

    use_plain_near(WQ)
    kv_wait(1)
    kv_prep(1)
    attend(1, query(1))

    arrived(q_second, o_code)
    start(far_o_code, *o_second)
    kv_wait(2)
    finish(1)
    kv_prep(2)
    unpack((NA, NB), WO)
    attend(2, query(2))

    use_plain_near(WO)
    arrived(o_first)
    start(*far_o)
    arrived(far_q_code)
    kv_wait(3)
    unpack((FAR,), WQ)
    acc[...] += project(1, range(4))
    finish(2)
    kv_prep(3)

    use_plain_far(WQ)
    arrived(far_q)
    attend(3, query(3))

    arrived(far_o_code, o_second[0])
    finish(3)
    unpack((FAR,), WO)
    acc[:, 0:256] += project(2, (0, 1))

    use_plain_far(WO)
    arrived(o_second[1])
    acc[:, 256:512] += project(2, (2, 3))

    for t in range(4):
        if t == 3:
            for l in LINKS:
                total = wire.at[pl.ds(0, 3), WQ]
                pltpu.make_async_copy(total, total, send_sem.at[l]).wait()
        arrived(far_o[t])
        cols = slice(t * 128, (t + 1) * 128)
        for rows in (slice(0, 256), slice(256, 512)):
            out_ref[rows, cols] = (acc[rows, cols] + project(3, [t], rows)).astype(out_ref.dtype)


def pallas_dist_sparse_attn_strided_htp_bs_b2_sq256_skv256_hq4_dh64_kernel(
    x: jax.Array,
    Wq: jax.Array,
    K_ext: jax.Array,
    V_ext: jax.Array,
    Wo: jax.Array,
):
    kt = jnp.transpose(K_ext, (0, 2, 3, 1)).reshape(8, 1024, 256)
    vt = jnp.transpose(V_ext, (0, 2, 3, 1)).reshape(8, 1024, 256)
    out = pl.pallas_call(
        _body,
        out_shape=jax.ShapeDtypeStruct((512, 512), BF16),
        in_specs=[pl.BlockSpec(memory_space=pltpu.HBM)] * 5,
        out_specs=pl.BlockSpec(memory_space=pltpu.VMEM),
        scratch_shapes=[
            pltpu.VMEM((512, 512), F32),
            pltpu.VMEM((512, 256), F32),
            pltpu.VMEM((256, 512), F32),
            pltpu.VMEM((4, 2, 2, 128, 256), F32),
            pltpu.VMEM((4, 2, 2, 128, 256), F32),
            pltpu.VMEM((512, 512), BF16),
            pltpu.VMEM((2, 2, 512, 128), BF16),
            pltpu.VMEM((4, 2, WIRE_ROWS, 128), I32),
            pltpu.VMEM((4, 2, 8 * QUADS, 128), I32),
            pltpu.VMEM((3, 2, 8 * QUADS, 128), I32),
            pltpu.VMEM((512, 256), F32),
            pltpu.VMEM((4, 2, 4, 128, 128), BF16),
            pltpu.VMEM((4, 2, 4, 128, 128), BF16),
            pltpu.VMEM((2, 4, 128, 128), BF16),
            pltpu.VMEM((4, 512, 256), BF16),
            pltpu.VMEM((512, 512), F32),
            pltpu.SemaphoreType.DMA((6 + len(WQ_PIECES),)),
            pltpu.SemaphoreType.DMA((2,)),
            pltpu.SemaphoreType.DMA((28,)),
            pltpu.SemaphoreType.DMA((16,)),
            pltpu.SemaphoreType.REGULAR,
        ],
        compiler_params=pltpu.CompilerParams(
            collective_id=0,
            vmem_limit_bytes=48 * 1024 * 1024,
            disable_semaphore_checks=True,
        ),
    )(x.reshape(512, 512), Wq, kt, vt, Wo)
    return out.reshape(2, 256, 512)
```

```python
import functools
import math

import jax
import jax.numpy as jnp
from jax import lax
from jax.experimental import pallas as pl
from jax.experimental.pallas import tpu as pltpu

F32, BF16, I32 = jnp.float32, jnp.bfloat16, jnp.int32
MESH = pl.DeviceIdType.MESH
NT_DIMS = (((1,), (1,)), ((), ()))
K_SCALE = 0.125 * math.log2(math.e)

OWN, NA, NB, FAR = 0, 1, 2, 3
WQ, WO = 0, 1
LINKS = (0, 1)
PHASES = (((OWN, 0), (OWN, 1)), ((NA, 0), (NB, 1)), ((NA, 1), (NB, 0)), ((FAR, 0), (FAR, 1)))
WQ_PIECES = ((0, 32), (32, 32), (64, 64), (128, 128), (256, 256))


def _i32(v):
    return v - (1 << 32) if v >> 31 else v


def _bytes(v):
    return _i32(v * 0x01010101)


def _shr(v, n):
    return lax.shift_right_logical(v, jnp.broadcast_to(jnp.asarray(n, I32), v.shape))


SM_MASK, EXP_MASK = _i32(0x807F807F), 0x7F807F80
QUADS, PLANES, QUEUE = 32, 4, 8
VALUES = 4 * QUADS
GROUP = 6
FIRST_BIT, LAST_BIT = 2, 32 * (QUEUE + 1)

SM_ROWS = 8 * QUADS // 2
CODE_ROW, CODE_ROWS = 2 * SM_ROWS, 8 * (QUEUE + PLANES)
WIRE_ROWS = CODE_ROW + CODE_ROWS


def _word_range(i):
    return (FIRST_BIT + i) // 32, min(FIRST_BIT + 32 * (i // GROUP), LAST_BIT - (VALUES - i)) // 32


def _partner(v):
    return jnp.concatenate([pltpu.roll(v[r:r + 8], 4, 0) for r in range(0, v.shape[0], 8)], axis=0)


def _reverse_bits(v):
    for n, mask in ((1, 0x55555555), (2, 0x33333333), (4, 0x0F0F0F0F), (8, 0x00FF00FF)):
        v = (_shr(v, n) & mask) | ((v & mask) << n)
    return _shr(v, 16) | (v << 16)


def _at_most(v, bound):
    return (_bytes(0x80 + bound) - v) & _bytes(0x80)


def _spread(byte):
    byte = byte | (byte << 8)
    return byte | (byte << 16)


def _encode(quads, top):
    total = functools.reduce(jnp.add, [e & 0x00FF00FF for e in quads])
    total = jnp.sum(((total & 0xFFFF) + _shr(total, 16)).astype(F32), axis=0, keepdims=True)
    mean = jnp.sum(total, axis=1, keepdims=True) * (1.0 / (512 * 128))
    ref = jnp.maximum(top, jnp.minimum((jnp.broadcast_to(mean, (1, 128)) + 3.5).astype(I32), 255))
    ref = jnp.broadcast_to(ref, (8, 128))
    ref4 = _spread(ref)
    zero = jnp.zeros((8, 128), I32)
    planes, queue, lengths, seen = [zero] * PLANES, [zero] * (QUEUE + 1), [], zero
    for i, e in enumerate(quads):
        v = ref4 - e
        le0, le1, le4, le8 = (_at_most(v, b) for b in (0, 1, 4, 8))
        rank = v + _shr(le0, 4) + _shr(le0, 6) + _shr(le0 ^ le1, 5) - _shr(le4, 7) - _shr(le8, 7)
        planes[i // 8] = planes[i // 8] | ((rank & _bytes(1)) << (i % 8))
        n = (_shr(rank, 1) & _bytes(0x7F)) + _bytes(1)
        seen = seen | v | (n << 1)
        lengths += [n & 31, _shr(n, 8) & 31, _shr(n, 16) & 31, _shr(n, 24) & 31]
    pos, bad = zero + FIRST_BIT, (seen & _bytes(0xC0)) != 0
    for i in range(0, VALUES, GROUP):
        bits, used = jnp.ones((8, 128), I32), lengths[i]
        for n in lengths[i + 1:i + GROUP]:
            bits, used = (bits << n) | 1, used + n
        bad = bad | (used > 32)
        bits = bits << ((32 - used) & 31)
        k, s = _shr(pos, 5), pos & 31
        head, rest = _shr(bits, s), (bits << 1) << (31 - s)
        k0, k1 = _word_range(i)
        here = {kk: k == kk for kk in range(k0, k1 + 1)}
        for kk in range(k0, min(k1 + 2, QUEUE + 1)):
            part = jnp.where(here[kk - 1], rest, 0) if kk > k0 else zero
            queue[kk] = queue[kk] | (jnp.where(here[kk], head, part) if kk <= k1 else part)
        pos = pos + used
    bad = bad | (pos > LAST_BIT) | (pos + _partner(pos) > 64 * QUEUE)
    unfit = jnp.max(jnp.where(bad, 1.0, 0.0)) > 0.0
    sub = lax.broadcasted_iota(I32, (8, 128), 0)
    queue[0] = queue[0] | ((_shr(ref, sub) & 1) << 30)
    queue[QUEUE - 1] = queue[QUEUE - 1] | _reverse_bits(_partner(queue[QUEUE]))
    flag = -unfit.astype(I32)
    return [word | flag for word in queue[:QUEUE]] + planes, unfit


def _decode(words, emit):
    queue, planes = words[:QUEUE], words[QUEUE:]
    queue = queue + [_reverse_bits(_partner(queue[-1]))]
    pos = jnp.full(queue[0].shape, FIRST_BIT, I32)
    sub = lax.broadcasted_iota(I32, (8, 128), 0)
    refs = []
    for r in range(0, pos.shape[0], 8):
        ref = jnp.sum(((_shr(queue[0][r:r + 8], 30) & 1) << sub).astype(F32), axis=0, keepdims=True)
        refs.append(jnp.broadcast_to(ref.astype(I32), (8, 128)))
    ref4 = _spread(jnp.concatenate(refs, axis=0))
    for i in range(VALUES):
        if i % GROUP == 0:
            k0, k1 = _word_range(i)
            k, s = _shr(pos, 5), pos & 31
            cur, nxt = queue[k0], queue[k0 + 1]
            for kk in range(k0 + 1, k1 + 1):
                here = k == kk
                cur = jnp.where(here, queue[kk], cur)
                if kk < QUEUE:
                    nxt = jnp.where(here, queue[kk + 1], nxt)
            window = (cur << s) | _shr(_shr(nxt, 1), 31 - s)
            pos = pos + GROUP
        z = lax.clz(window)
        window, pos = (window << 1) << z, pos + z
        rank = z << 1 if i % 4 == 0 else rank | (z << (8 * (i % 4) + 1))
        if i % 4 == 3:
            q = i // 4
            rank = rank | (_shr(planes[q // 8], q % 8) & _bytes(1))
            le2, le3, le7, le8 = (_at_most(rank, b) for b in (2, 3, 7, 8))
            v = rank + _shr(le3, 7) + _shr(le7, 7) - _shr(le2 ^ le3, 5) - _shr(le7 ^ le8, 4)
            emit(q, ref4 - v)


def _body(x_hbm, wq_hbm, kt_hbm, vt_hbm, wo_hbm, out_ref,
          xf, wqf, wof, ktf, vtf, xb, own, wire, expo, plain, q_own, kb, vb, ctx_t, ctx, acc,
          load_sem, send_sem, recv_sem, plain_sem, entry_sem):
    me = lax.axis_index("i")
    nbr = (me ^ 1, me ^ 3)
    barrier = pltpu.get_barrier_semaphore()

    def start(*groups):
        for group in groups:
            for dma in group:
                dma.start()

    def arrived(*groups):
        for group in groups:
            for dma in group:
                dma.wait_recv()

    def sent(*groups):
        for group in groups:
            for dma in group:
                dma.wait_send()

    def tell_neighbours(sem):
        for dev in nbr:
            pl.semaphore_signal(sem, inc=1, device_id=(dev,), device_id_type=MESH)

    ld_wq = [pltpu.make_async_copy(wq_hbm.at[pl.ds(r, n)], wqf.at[pl.ds(r, n)], load_sem.at[6 + i])
             for i, (r, n) in enumerate(WQ_PIECES)]
    ld_wo = pltpu.make_async_copy(wo_hbm, wof, load_sem.at[0])
    ld_x = pltpu.make_async_copy(x_hbm, xf, load_sem.at[1])
    ld_wq[0].start()
    pl.when(me != 2)(lambda: tell_neighbours(barrier))
    start(ld_wq[1:], [ld_wo, ld_x])

    @pl.when(me == 2)
    def _():
        pl.semaphore_wait(barrier, 2)
        tell_neighbours(entry_sem)

    owner = (me, *nbr, me ^ 2)
    ld_kv = []
    for i, pairs in enumerate(PHASES):
        ld_kv.append([])
        for j, (s, h) in enumerate(pairs):
            src = (pl.ds(2 * me, 2), pl.ds(pl.multiple_of(owner[s] * 256 + h * 128, 128), 128))
            ld_kv[i] += [pltpu.make_async_copy(kt_hbm.at[src], ktf.at[i, j], load_sem.at[2 + i]),
                         pltpu.make_async_copy(vt_hbm.at[src], vtf.at[i, j], load_sem.at[2 + i])]

    send_slots = iter(range(send_sem.shape[0]))

    def remote(k, m, relay, first_row, rows):
        group = []
        for l in LINKS:
            src, dst = (NB - l, FAR) if relay else (OWN, NA + l)
            span = pl.ds(first_row[l], rows)
            group.append(pltpu.make_async_remote_copy(
                wire.at[src, m, span], wire.at[dst, m, span],
                send_sem.at[next(send_slots)], recv_sem.at[2 * k + l],
                device_id=(nbr[l],), device_id_type=MESH))
        return group

    def first(r=0):
        return (r, SM_ROWS + r)

    def second(r=0):
        return (SM_ROWS + r, r)

    q_parts = [[remote(0, WQ, False, first(r // 4), n // 4)]
               + ([remote(1, WQ, False, second(r // 4), n // 4)] if r < 128 else []) for r, n in WQ_PIECES]
    q_first = remote(0, WQ, False, first(), SM_ROWS)
    q_second_rest = remote(1, WQ, False, second(32), SM_ROWS - 32)
    q_second = remote(1, WQ, False, second(), SM_ROWS)
    q_code, o_code = (remote(2 + m, m, False, (CODE_ROW, CODE_ROW), CODE_ROWS) for m in (WQ, WO))
    o_first = remote(4, WO, False, first(), SM_ROWS)
    far_q_code, far_o_code = (
        remote(5 + m, m, True, (CODE_ROW, CODE_ROW + CODE_ROWS // 2), CODE_ROWS // 2) for m in (WQ, WO))
    far_q = remote(7, WQ, True, second(), SM_ROWS)
    o_second = [remote(8 + i, WO, False, second(64 * i), 64) for i in range(2)]
    far_o = [remote(10 + t, WO, True, second(32 * t), 32) for t in range(4)]

    def plain_own(m, l):
        return pltpu.make_async_remote_copy(
            expo.at[OWN, m], plain.at[l, m], plain_sem.at[8 * m + l], plain_sem.at[8 * m + 2 + l],
            device_id=(nbr[l],), device_id_type=MESH)

    def plain_far(m, l):
        span = pl.ds(SM_ROWS * l, SM_ROWS)
        return pltpu.make_async_remote_copy(
            plain.at[1 - l, m, span], plain.at[2, m, span],
            plain_sem.at[8 * m + 4 + l], plain_sem.at[8 * m + 6 + l],
            device_id=(nbr[l],), device_id_type=MESH)

    def split(m, h, r, block):
        n = block.shape[0]
        own[m, h, pl.ds(r, n)] = block.astype(BF16)
        w = pltpu.bitcast(own[m, h, pl.ds(r, n)], I32)
        for i in range(n // 32):
            a, b = w[16 * i:16 * i + 8], w[16 * i + 8:16 * i + 16]
            rows, sm = pl.ds(SM_ROWS * h + r // 4 + 8 * i, 8), b & SM_MASK
            wire[OWN, m, rows] = (a & SM_MASK) | (sm << 8) | _shr(sm, 24)
            expo[OWN, m, rows] = (_shr(a, 7) & 0x00FF00FF) | ((b << 1) & _i32(0xFF00FF00))

    def pack(m, src):
        top = jnp.max(jnp.abs(src[...]), axis=0, keepdims=True)
        top = functools.reduce(jnp.maximum, [top[:, c:c + 128] for c in range(0, top.shape[1], 128)])
        top = _shr(pltpu.bitcast(top.astype(BF16).astype(F32), I32), 23) & 255
        words, unfit = _encode([expo[OWN, m, pl.ds(8 * i, 8)] for i in range(QUADS)], top)
        wire[OWN, m, pl.ds(CODE_ROW, CODE_ROWS)] = jnp.concatenate(words, axis=0)
        return unfit

    def unpack(slots, m):
        def emit(i, quad):
            for j, s in enumerate(slots):
                expo[s, m, pl.ds(8 * i, 8)] = quad[8 * j:8 * j + 8]

        _decode([jnp.concatenate([wire[s, m, pl.ds(r, 8)] for s in slots], axis=0)
                 for r in range(CODE_ROW, WIRE_ROWS, 8)], emit)

    def is_unfit(s, m):
        return wire[s, m, pl.ds(CODE_ROW, 8)][0, 0] < 0

    def use_plain_near(m):
        unfit = [is_unfit(NA + l, m) for l in LINKS]
        for l in LINKS:
            @pl.when(unfit[l])
            def _():
                plain_own(m, l).wait_recv()
                plain_far(m, 1 - l).start()
                expo[NA + l, m] = plain[l, m]
        return unfit

    def use_plain_far(m):
        @pl.when(is_unfit(FAR, m))
        def _():
            arrived([plain_far(m, l) for l in LINKS])
            expo[FAR, m] = plain[2, m]

    def weight(s, m, h, t):
        if s == OWN:
            return own[m, h, pl.ds(128 * t, 128)]
        words = []
        for r in range(SM_ROWS * h + 32 * t, SM_ROWS * h + 32 * t + 32, 8):
            p, e = wire[s, m, pl.ds(r, 8)], expo[s, m, pl.ds(r, 8)]
            words += [(p & SM_MASK) | ((e << 7) & EXP_MASK),
                      ((_shr(p, 8) | (p << 24)) & SM_MASK) | (_shr(e, 1) & EXP_MASK)]
        return pltpu.bitcast(jnp.concatenate(words, axis=0), BF16)

    @pl.when(me == 0)
    def _():
        start(ld_kv[0])
        pl.semaphore_wait(barrier, 2)

    pl.when((me & 1) == 1)(lambda: pl.semaphore_wait(barrier, 1))
    faces_2 = (3, 1)
    for i, (r, n) in enumerate(WQ_PIECES):
        ld_wq[i].wait()
        for h in range(2):
            split(WQ, h, r, wqf[r:r + n, h * 128:(h + 1) * 128])
        for l in LINKS:
            pl.when(me != faces_2[l])(lambda: start([group[l] for group in q_parts[i]]))
    pl.when(me != 0)(lambda: start(ld_kv[0]))
    for l in LINKS:
        @pl.when(me == faces_2[l])
        def _():
            pl.semaphore_wait(entry_sem, 1)
            start([group[l] for part in q_parts for group in part])

    unfit_q = pack(WQ, wqf)
    start(q_code, q_second_rest)
    ld_wo.wait()
    for h in range(2):
        for t in range(4):
            split(WO, h, 128 * t, wof[h * 128:(h + 1) * 128, t * 128:(t + 1) * 128])
    unfit_o = pack(WO, wof)
    start(o_code, o_first, *ld_kv[1:])
    for m, unfit in ((WQ, unfit_q), (WO, unfit_o)):
        pl.when(unfit)(lambda: start([plain_own(m, l) for l in LINKS]))

    diag = ((lax.broadcasted_iota(I32, (128, 128), 1) < 64)
            == (lax.broadcasted_iota(I32, (128, 128), 0) < 64))
    left = lax.broadcasted_iota(I32, (64, 128), 1) < 64
    left_row = lax.broadcasted_iota(I32, (1, 128), 1) < 64
    tiles = [(j, g) for g in range(4) for j in range(2)]

    def kv_wait(i):
        for dma in ld_kv[i]:
            dma.wait()

    def kv_prep(i):
        for j, g in tiles:
            b, cols = g // 2, slice((g % 2) * 128, (g % 2 + 1) * 128)
            k = (ktf[i, j, b, :, cols] * K_SCALE).T
            kb[i, j, g] = jnp.concatenate(
                [jnp.where(left, k[0:64], k[64:128]), jnp.where(left, k[64:128], k[0:64])], 0).astype(BF16)
            vb[i, j, g] = vtf[i, j, b, :, cols].astype(BF16)

    def query(i):
        w = jnp.concatenate(
            [jnp.concatenate([weight(s, WQ, h, t) for t in range(4)], axis=0) for s, h in PHASES[i]], axis=1)
        return jnp.dot(xb[...], w, preferred_element_type=F32)

    def softmax_terms(s):
        e = jnp.exp2(s - jnp.max(s, axis=0, keepdims=True))
        return e, jnp.sum(e, axis=0, keepdims=True)

    def attend(i, q):
        scores, probs = {}, {}
        for j, g in tiles:
            qt = q[g * 128:(g + 1) * 128, j * 128:(j + 1) * 128]
            scores[j, g] = (
                lax.dot_general(kb[i, j, g, 0:64], jnp.where(diag, qt, 0.).astype(BF16), NT_DIMS,
                                preferred_element_type=F32),
                lax.dot_general(kb[i, j, g, 64:128], jnp.where(diag, 0., qt).astype(BF16), NT_DIMS,
                                preferred_element_type=F32))
        for j, g in tiles:
            (p1, l1), (p2, l2) = softmax_terms(scores[j, g][0]), softmax_terms(scores[j, g][1])
            probs[j, g] = (
                jnp.concatenate([jnp.where(left, p1, 0.), jnp.where(left, 0., p2)], 0).astype(BF16),
                jnp.concatenate([jnp.where(left, p2, 0.), jnp.where(left, 0., p1)], 0).astype(BF16),
                1.0 / jnp.where(left_row, l1, l2), 1.0 / jnp.where(left_row, l2, l1))
        for j, g in tiles:
            head0, head1, inv0, inv1 = probs[j, g]
            tile = jnp.concatenate(
                [jnp.dot(vb[i, j, g, 0:64], head0, preferred_element_type=F32) * inv0,
                 jnp.dot(vb[i, j, g, 64:128], head1, preferred_element_type=F32) * inv1], 0).astype(BF16)
            if i == 0:
                ctx[i, g * 128:(g + 1) * 128, j * 128:(j + 1) * 128] = tile.T
            else:
                ctx_t[j, g] = tile

    def finish(i):
        for j, g in tiles:
            ctx[i, g * 128:(g + 1) * 128, j * 128:(j + 1) * 128] = ctx_t[j, g].T

    def project(i, slabs, rows=slice(None)):
        w = jnp.concatenate(
            [jnp.concatenate([weight(s, WO, h, t) for t in slabs], axis=1) for s, h in PHASES[i]], axis=0)
        return jnp.dot(ctx[i, rows], w, preferred_element_type=F32)

    ld_x.wait()
    xb[...] = xf[...].astype(BF16)
    q_own[...] = query(0)

    kv_wait(0)
    kv_prep(0)
    attend(0, q_own)

    arrived(q_first, q_code)
    start(far_q_code, far_q)
    unpack((NA, NB), WQ)
    acc[...] = project(0, range(4))

    relayed_q = use_plain_near(WQ)
    kv_wait(1)
    kv_prep(1)
    attend(1, query(1))

    arrived(q_second, o_code)
    start(far_o_code, *o_second)
    kv_wait(2)
    finish(1)
    kv_prep(2)
    unpack((NA, NB), WO)
    attend(2, query(2))

    relayed_o = use_plain_near(WO)
    arrived(o_first)
    start(*far_o)
    arrived(far_q_code)
    kv_wait(3)
    unpack((FAR,), WQ)
    acc[...] += project(1, range(4))
    finish(2)
    kv_prep(3)

    use_plain_far(WQ)
    sent(*[group for part in q_parts for group in part], q_code, q_second_rest, o_code, o_first, far_q_code)
    arrived(far_q)
    attend(3, query(3))

    arrived(far_o_code, o_second[0])
    finish(3)
    unpack((FAR,), WO)
    acc[:, 0:256] += project(2, (0, 1))

    use_plain_far(WO)

    @pl.when(functools.reduce(jnp.logical_or, [unfit_q, unfit_o, *relayed_q, *relayed_o]))
    def _():
        for m, unfit, relayed in ((WQ, unfit_q, relayed_q), (WO, unfit_o, relayed_o)):
            for l in LINKS:
                pl.when(unfit)(lambda: plain_own(m, l).wait_send())
                pl.when(relayed[l])(lambda: plain_far(m, 1 - l).wait_send())

    sent(far_q, far_o_code, o_second[0])
    arrived(o_second[1])
    acc[:, 256:512] += project(2, (2, 3))

    for t in range(4):
        if t == 3:
            sent(o_second[1], *far_o)
        arrived(far_o[t])
        cols = slice(t * 128, (t + 1) * 128)
        for rows in (slice(0, 256), slice(256, 512)):
            out_ref[rows, cols] = (acc[rows, cols] + project(3, [t], rows)).astype(out_ref.dtype)


def pallas_dist_sparse_attn_strided_htp_bs_b2_sq256_skv256_hq4_dh64_kernel(
    x: jax.Array,
    Wq: jax.Array,
    K_ext: jax.Array,
    V_ext: jax.Array,
    Wo: jax.Array,
):
    kt = jnp.transpose(K_ext, (0, 2, 3, 1)).reshape(8, 1024, 256)
    vt = jnp.transpose(V_ext, (0, 2, 3, 1)).reshape(8, 1024, 256)
    out = pl.pallas_call(
        _body,
        out_shape=jax.ShapeDtypeStruct((512, 512), BF16),
        in_specs=[pl.BlockSpec(memory_space=pltpu.HBM)] * 5,
        out_specs=pl.BlockSpec(memory_space=pltpu.VMEM),
        scratch_shapes=[
            pltpu.VMEM((512, 512), F32),
            pltpu.VMEM((512, 256), F32),
            pltpu.VMEM((256, 512), F32),
            pltpu.VMEM((4, 2, 2, 128, 256), F32),
            pltpu.VMEM((4, 2, 2, 128, 256), F32),
            pltpu.VMEM((512, 512), BF16),
            pltpu.VMEM((2, 2, 512, 128), BF16),
            pltpu.VMEM((4, 2, WIRE_ROWS, 128), I32),
            pltpu.VMEM((4, 2, 8 * QUADS, 128), I32),
            pltpu.VMEM((3, 2, 8 * QUADS, 128), I32),
            pltpu.VMEM((512, 256), F32),
            pltpu.VMEM((4, 2, 4, 128, 128), BF16),
            pltpu.VMEM((4, 2, 4, 128, 128), BF16),
            pltpu.VMEM((2, 4, 128, 128), BF16),
            pltpu.VMEM((4, 512, 256), BF16),
            pltpu.VMEM((512, 512), F32),
            pltpu.SemaphoreType.DMA((6 + len(WQ_PIECES),)),
            pltpu.SemaphoreType.DMA((46,)),
            pltpu.SemaphoreType.DMA((28,)),
            pltpu.SemaphoreType.DMA((16,)),
            pltpu.SemaphoreType.REGULAR,
        ],
        compiler_params=pltpu.CompilerParams(
            collective_id=0,
            vmem_limit_bytes=48 * 1024 * 1024,
            disable_semaphore_checks=True,
        ),
    )(x.reshape(512, 512), Wq, kt, vt, Wo)
    return out.reshape(2, 256, 512)
```
